```python
import numpy as np

kernel_name = "dist_sparse_attn_strided_htp_bs_b2_sq256_skv256_hq4_dh64"

def setup_inputs():
    x = np.random.randn(8, 256, 512).astype(np.float32)
    Wq = np.random.randn(512, 1024).astype(np.float32) * 0.02
    K_ext = np.random.randn(8, 256, 16, 64).astype(np.float32)
    V_ext = np.random.randn(8, 256, 16, 64).astype(np.float32)
    Wo = np.random.randn(1024, 512).astype(np.float32) * 0.02
    return {"x": x, "Wq": Wq, "K_ext": K_ext, "V_ext": V_ext, "Wo": Wo}

def reference(x, Wq, K_ext, V_ext, Wo):
    B, Sq, Skv, Hq, Dh = 8, 256, 256, 16, 64
    Q = (x @ Wq).reshape(B, Sq, Hq, Dh)
    qb = (np.arange(Sq) // 64)[:, None]
    kb = (np.arange(Skv) // 64)[None, :]
    mask = (qb == kb) | ((kb % 4) == (qb % 4))
    scores = np.einsum('bihd,bjhd->bhij', Q, K_ext).astype(np.float32) * 0.125
    scores = np.where(mask[None, None, :, :], scores, -1e9)
    scores_max = scores.max(axis=-1, keepdims=True)
    w = np.exp(scores - scores_max)
    row_keep = mask.any(axis=1)
    w_sum = np.where(row_keep[None, None, :, None], w.sum(axis=-1, keepdims=True), 1.0)
    w = w / w_sum
    w = np.where(row_keep[None, None, :, None], w, 0.0)
    ctx = np.einsum('bhij,bjhd->bihd', w, V_ext).reshape(B, Sq, Hq * Dh)
    return ctx @ Wo
```

```python
import contextlib
import math

import jax
import jax.numpy as jnp
from jax import lax
from jax.experimental import pallas as pl
from jax.experimental.pallas import tpu as pltpu

TRACE = False
OUT_DTYPE = jnp.bfloat16
NO_SEM_CHECKS = True

N_DEV = 4
B_LOC = 2
SEQ = 256
D_MODEL = 512
TOK = B_LOC * SEQ
BLK = 64
PAIR = 128
LOG2E = math.log2(math.e)
SCORE_SCALE = 0.125 * LOG2E
MASKED_SCORE = -1e9 * LOG2E

OWN, LEFT, RIGHT, DIAG = range(4)
WQ_ROW_CUTS = (0, 32, 128, 512)

BF16 = jnp.bfloat16
F32 = jnp.float32


def _scope(name):
    return jax.named_scope("T_" + name) if TRACE else contextlib.nullcontext()


def _body(x_hbm, wq_hbm, kt_hbm, vt_hbm, wo_hbm, out_ref,
          x_f32, wq_f32, wo_f32, k_f32, v_f32,
          xb, wq_all, wo_all, ctx, acc,
          wq_sem, wo_sem, x_sem, kv_sem, send_sem, recv_sem, last_sem, ready_sem):
    me = lax.axis_index("i")
    left = (me + 3) & 3
    right = (me + 1) & 3
    diag = (me + 2) & 3
    odd = (me & 1) == 1
    n_cuts = len(WQ_ROW_CUTS) - 1

    def signal(sem, dev):
        pl.semaphore_signal(sem, 1, device_id=(dev,), device_id_type=pl.DeviceIdType.MESH)

    def remote(src, dst, rsem, dev):
        return pltpu.make_async_remote_copy(
            src, dst, send_sem, rsem, device_id=(dev,), device_id_type=pl.DeviceIdType.MESH)

    wq_loads = []
    for c in range(n_cuts):
        rows = pl.ds(WQ_ROW_CUTS[c], WQ_ROW_CUTS[c + 1] - WQ_ROW_CUTS[c])
        wq_loads.append(pltpu.make_async_copy(wq_hbm.at[rows], wq_f32.at[rows], wq_sem.at[c]))
        wq_loads[-1].start()

    bar = pltpu.get_barrier_semaphore()

    @pl.when(me != 2)
    def _():
        signal(bar, left)
        signal(bar, right)

    wo_load = pltpu.make_async_copy(wo_hbm, wo_f32, wo_sem)
    wo_load.start()
    x_load = pltpu.make_async_copy(x_hbm, x_f32, x_sem)
    x_load.start()
    kv_loads = {}
    for slot, dev in ((OWN, me), (LEFT, left), (RIGHT, right), (DIAG, diag)):
        src = (pl.ds(me * B_LOC, B_LOC), pl.ds(pl.multiple_of(dev * 2 * PAIR, 2 * PAIR), 2 * PAIR))
        kv_loads[slot] = (
            pltpu.make_async_copy(kt_hbm.at[src], k_f32.at[slot], kv_sem.at[slot]),
            pltpu.make_async_copy(vt_hbm.at[src], v_f32.at[slot], kv_sem.at[slot]))

    def cast_wq(c):
        rows = pl.ds(WQ_ROW_CUTS[c], WQ_ROW_CUTS[c + 1] - WQ_ROW_CUTS[c])
        wq_loads[c].wait()
        for h in range(2):
            wq_all[OWN, h, rows, :] = wq_f32[rows, h * PAIR:(h + 1) * PAIR].astype(BF16)

    def send_wq_first(d, c):
        rows = pl.ds(WQ_ROW_CUTS[c], WQ_ROW_CUTS[c + 1] - WQ_ROW_CUTS[c])
        remote(wq_all.at[OWN, d, rows], wq_all.at[LEFT + d, d, rows], recv_sem.at[d],
               (right, left)[d]).start()

    with _scope("head"):
        @pl.when(odd)
        def _():
            pl.semaphore_wait(bar, 1)
            for c in range(n_cuts):
                cast_wq(c)
                pl.when(me == 3)(lambda: send_wq_first(0, c))
                pl.when(me == 1)(lambda: send_wq_first(1, c))
            pl.semaphore_wait(ready_sem, 1)
            for c in range(n_cuts):
                pl.when(me == 3)(lambda: send_wq_first(1, c))
                pl.when(me == 1)(lambda: send_wq_first(0, c))

        @pl.when(jnp.logical_not(odd))
        def _():
            pl.semaphore_wait(bar, 2)

            @pl.when(me == 2)
            def _():
                signal(ready_sem, left)
                signal(ready_sem, right)

            for c in range(n_cuts):
                cast_wq(c)
                send_wq_first(0, c)
                send_wq_first(1, c)

    for slot in range(4):
        for cp in kv_loads[slot]:
            cp.start()

    for d, dev in ((0, right), (1, left)):
        remote(wq_all.at[OWN, 1 - d], wq_all.at[LEFT + d, 1 - d], recv_sem.at[2 + d], dev).start()

    with _scope("wo"):
        wo_load.wait()
        for h in range(2):
            for n in range(4):
                wo_all[OWN, h, n] = wo_f32[h * PAIR:(h + 1) * PAIR, n * 128:(n + 1) * 128].astype(BF16)
        for d, dev in ((0, right), (1, left)):
            remote(wo_all.at[OWN, d], wo_all.at[LEFT + d, d], recv_sem.at[4 + d], dev).start()

    with _scope("x"):
        x_load.wait()
        for b in range(B_LOC):
            xb[b * SEQ:(b + 1) * SEQ, :] = x_f32[b].astype(BF16)

    lane = lax.broadcasted_iota(jnp.int32, (BLK, PAIR), 1)
    low = lane < BLK
    low2 = lax.broadcasted_iota(jnp.int32, (PAIR, PAIR), 1) < BLK

    def attention(pairs):
        w = jnp.concatenate([wq_all[s, h] for s, h in pairs], axis=1)
        q_all = jnp.dot(xb[...], w, preferred_element_type=F32).astype(BF16)
        for i, (s, h) in enumerate(pairs):
            for m in range(TOK // PAIR):
                b, t = divmod(m, SEQ // PAIR)
                q = q_all[m * PAIR:(m + 1) * PAIR, i * PAIR:(i + 1) * PAIR]
                k = (k_f32[s, b, h * PAIR:(h + 1) * PAIR, t * PAIR:(t + 1) * PAIR] * SCORE_SCALE).T
                kk = jnp.concatenate([jnp.where(low2, k, 0.0), jnp.where(low2, 0.0, k)], axis=0)
                st = lax.dot_general(kk.astype(BF16), q, (((1,), (1,)), ((), ())),
                                     preferred_element_type=F32)
                outs = []
                for e in range(2):
                    sc = jnp.where(low, st[e * PAIR:e * PAIR + BLK], st[e * PAIR + BLK:(e + 1) * PAIR])
                    mx = jnp.maximum(jnp.max(sc, axis=0, keepdims=True), MASKED_SCORE)
                    p = jnp.exp2(sc - mx)
                    pm = jnp.exp2(MASKED_SCORE - mx)
                    den = jnp.sum(p, axis=0, keepdims=True) + (SEQ - BLK) * pm
                    near = jnp.concatenate([jnp.where(low, p, pm), jnp.where(low, pm, p)], axis=0)
                    far = jnp.broadcast_to(pm, (PAIR, PAIR))
                    pt = jnp.concatenate([near, far] if t == 0 else [far, near], axis=0).astype(BF16)
                    v = v_f32[s, b, h * PAIR + e * BLK:h * PAIR + (e + 1) * BLK, :].astype(BF16)
                    o = jnp.dot(v, pt, preferred_element_type=F32)
                    outs.append(o * (1.0 / den))
                ctx[s, h, m * PAIR:(m + 1) * PAIR, :] = jnp.concatenate(outs, axis=0).T.astype(BF16)

    def out_proj(pairs, n_tiles):
        a = jnp.concatenate([ctx[s, h] for s, h in pairs], axis=1)
        w = jnp.concatenate(
            [jnp.concatenate([wo_all[s, h, n] for n in n_tiles], axis=1) for s, h in pairs], axis=0)
        return jnp.dot(a, w, preferred_element_type=F32)

    def wait_recv(buf, sem):
        pltpu.make_async_copy(buf, buf, sem).wait()

    with _scope("kv0"):
        for cp in kv_loads[OWN]:
            cp.wait()
    with _scope("att0"):
        attention([(OWN, 0), (OWN, 1)])

    with _scope("w1"):
        for d, dev in ((0, right), (1, left)):
            wait_recv(wq_all.at[LEFT + d, d], recv_sem.at[d])
            remote(wq_all.at[LEFT + d, d], wq_all.at[DIAG, d], recv_sem.at[6 + d], dev).start()
            remote(wo_all.at[OWN, 1 - d], wo_all.at[LEFT + d, 1 - d], recv_sem.at[8 + d], dev).start()
        for slot in (LEFT, RIGHT):
            for cp in kv_loads[slot]:
                cp.wait()
    with _scope("att1"):
        attention([(LEFT, 0), (RIGHT, 1)])

    with _scope("w2"):
        for d in range(2):
            wait_recv(wq_all.at[LEFT + d, 1 - d], recv_sem.at[2 + d])
    with _scope("att2"):
        attention([(LEFT, 1), (RIGHT, 0)])

    with _scope("w3"):
        for d, dev in ((0, right), (1, left)):
            wait_recv(wo_all.at[LEFT + d, d], recv_sem.at[4 + d])
            for n in range(4):
                remote(wo_all.at[LEFT + d, d, n], wo_all.at[DIAG, d, n], last_sem.at[n], dev).start()
    with _scope("op3"):
        acc[...] = out_proj([(OWN, 0), (OWN, 1), (LEFT, 0), (RIGHT, 1)], range(4))

    with _scope("w4"):
        for d in range(2):
            wait_recv(wq_all.at[DIAG, d], recv_sem.at[6 + d])
        for cp in kv_loads[DIAG]:
            cp.wait()
    with _scope("att4"):
        attention([(DIAG, 0), (DIAG, 1)])

    with _scope("w5"):
        for d in range(2):
            wait_recv(wo_all.at[LEFT + d, 1 - d], recv_sem.at[8 + d])
    with _scope("op5"):
        acc[...] += out_proj([(LEFT, 1), (RIGHT, 0)], range(4))

    for n in range(4):
        with _scope(f"w6{n}"):
            if n == 3:
                wait_recv(wq_all.at[pl.ds(LEFT, 3)], send_sem)
                wait_recv(wo_all.at[pl.ds(LEFT, 3)], send_sem)
            wait_recv(wo_all.at[DIAG, :, n], last_sem.at[n])
        with _scope(f"op6{n}"):
            cols = slice(n * 128, (n + 1) * 128)
            res = (acc[:, cols] + out_proj([(DIAG, 0), (DIAG, 1)], [n])).astype(out_ref.dtype)
            for b in range(B_LOC):
                out_ref[b, :, cols] = res[b * SEQ:(b + 1) * SEQ]


def pallas_dist_sparse_attn_strided_htp_bs_b2_sq256_skv256_hq4_dh64_kernel(x, Wq, K_ext, V_ext, Wo):
    n_b, skv, n_h, dh = K_ext.shape
    kt = K_ext.transpose(0, 2, 3, 1).reshape(n_b, n_h * dh, skv)
    vt = V_ext.transpose(0, 2, 3, 1).reshape(n_b, n_h * dh, skv)
    hbm = pl.BlockSpec(memory_space=pltpu.HBM)
    return pl.pallas_call(
        _body,
        out_shape=jax.ShapeDtypeStruct(x.shape, OUT_DTYPE),
        in_specs=[hbm] * 5,
        out_specs=pl.BlockSpec(memory_space=pltpu.VMEM),
        scratch_shapes=[
            pltpu.VMEM((B_LOC, SEQ, D_MODEL), F32),
            pltpu.VMEM((D_MODEL, 2 * PAIR), F32),
            pltpu.VMEM((2 * PAIR, D_MODEL), F32),
            pltpu.VMEM((4, B_LOC, 2 * PAIR, SEQ), F32),
            pltpu.VMEM((4, B_LOC, 2 * PAIR, SEQ), F32),
            pltpu.VMEM((TOK, D_MODEL), BF16),
            pltpu.VMEM((4, 2, D_MODEL, PAIR), BF16),
            pltpu.VMEM((4, 2, 4, PAIR, 128), BF16),
            pltpu.VMEM((4, 2, TOK, PAIR), BF16),
            pltpu.VMEM((TOK, D_MODEL), F32),
            pltpu.SemaphoreType.DMA((len(WQ_ROW_CUTS) - 1,)),
            pltpu.SemaphoreType.DMA,
            pltpu.SemaphoreType.DMA,
            pltpu.SemaphoreType.DMA((4,)),
            pltpu.SemaphoreType.DMA,
            pltpu.SemaphoreType.DMA((10,)),
            pltpu.SemaphoreType.DMA((4,)),
            pltpu.SemaphoreType.REGULAR,
        ],
        compiler_params=pltpu.CompilerParams(
            collective_id=0, vmem_limit_bytes=48 * 1024 * 1024,
            disable_semaphore_checks=NO_SEM_CHECKS),
    )(x, Wq, kt, vt, Wo)
```

```python
import math

import jax
import jax.numpy as jnp
from jax import lax
from jax.experimental import pallas as pl
from jax.experimental.pallas import tpu as pltpu

BF16 = jnp.bfloat16
F32 = jnp.float32
I32 = jnp.int32

B_LOC = 2
SEQ = 256
D_MODEL = 512
TOK = B_LOC * SEQ
BLK = 64
PAIR = 128
LOG2E = math.log2(math.e)
SCORE_SCALE = 0.125 * LOG2E
MASKED_SCORE = -1e9 * LOG2E

OWN, LEFT, RIGHT, DIAG = range(4)
WQ, WO = range(2)
STEPS = (((OWN, 0), (OWN, 1)), ((LEFT, 0), (RIGHT, 1)), ((LEFT, 1), (RIGHT, 0)), ((DIAG, 0), (DIAG, 1)))

TILES = 32
BODY_TILES = 22
PLANE_TILES = 11
NOTE_ROWS = 5
LIST_MAX = 6
LANE_MAX = 19
HIGH = 0x7C007C00
REST = ~HIGH
LISTED = 0x0C000C00
HEAD_CUTS = (0, 3, 9, 16, 32)
LATE_CUTS = (0, 16, 32)
TAIL_CUTS = (0, 8, 16, 20, 24, 28, 32)


def _body_plan(w):
    plan = []
    for base in (0, 16):
        spread = [base + 3 * i + (3 if w == WO else 2) for i in range(5)]
        bits = [(t - 2 + i, [(t, 10 - 5 * i, HIGH)]) for t in spread for i in range(2)]
        signs = [(base if w == WO else base + 15,
                  [(t, -1 - i, 0x40004000 >> i) for i, t in enumerate(spread)])]
        plan += signs + bits if w == WO else bits + signs
    return plan


PLAN = (_body_plan(WQ), _body_plan(WO))


def _body_cut(w, n):
    return sum(kept < n for kept, _ in PLAN[w])


def _shr(v, n):
    return lax.shift_right_logical(*jnp.broadcast_arrays(v, jnp.asarray(n, I32)))


def _shift(v, n):
    return v if n == 0 else v << n if n > 0 else _shr(v, -n)


def _sublane():
    return lax.broadcasted_iota(I32, (8, 128), 0)


def _both_halves(row):
    return jnp.broadcast_to(row | (row << 16), (8, 128))


def _highest(rest, floor):
    return ((rest + (0x04000400 - (floor & 0x03FF03FF))) & REST) + floor


def _list_starts(counts):
    def total(v):
        v = (v & 0o07070707) + ((v >> 3) & 0o07070707)
        v = v + (v >> 12)
        return (v + (v >> 6)) & 63

    before = (1 << (3 * _sublane())) - 1
    return ([5 * total(counts[0] & before), 5 * (total(counts[0]) + total(counts[1] & before))],
            total(counts[0]) + total(counts[1]))


def _make_note(tiles):
    zero = jnp.zeros((8, 128), I32)
    largest = zero
    for v in tiles:
        largest = jnp.maximum(largest, jnp.maximum(v & 0x7FFF, (v >> 16) & 0x7FFF))
    floor = jnp.maximum(jnp.max(largest, axis=0, keepdims=True) - 0x3FF, 0)
    floors = _both_halves(floor)
    excess = [_highest(v & REST, floors) - v for v in tiles]
    fields = [zero] * 4
    unlisted = zero
    for t, v in enumerate(excess):
        fields[t // 8] |= _shift(v & LISTED, 2 * (t % 8) - 10)
        unlisted |= v
    unlisted &= ~LISTED
    lists, counts = [], []
    for a, b in (fields[:2], fields[2:]):
        entries = count = zero
        for _ in range(LIST_MAX):
            second = a == 0
            v = jnp.where(second, b, a)
            v = (v | (v >> 1)) & 0x55555555
            one = v & (0 - v)
            field = ((pltpu.bitcast(one.astype(F32), I32) >> 23) - 127) >> 1
            a, b = a - jnp.where(second, 0, one), b - jnp.where(second, one, 0)
            entries = jnp.where(v != 0, (entries << 5) | field | jnp.where(second, 16, 0), entries)
            count += jnp.where(v != 0, 1, 0)
        unlisted |= a | b
        lists.append(entries)
        counts.append(jnp.sum(count << (3 * _sublane()), axis=0, keepdims=True))
    starts, total = _list_starts(counts)
    rows = []
    for r in range(3):
        part = zero
        for entries, start in zip(lists, starts):
            part |= jnp.where(start >> 5 == r, entries << (start & 31), 0)
            part |= jnp.where(start >> 5 == r - 1, (entries >> 1) >> (31 - (start & 31)), 0)
        rows.append(jnp.sum(part, axis=0, keepdims=True))
    short = jnp.max(jnp.where((unlisted != 0) | (total > LANE_MAX), 1.0, 0.0)) > 0.0
    rows.append(counts[0] | (floor << 24))
    rows.append(counts[1] | ((floor >> 8) << 24) | (short.astype(I32) << 31))
    return rows, excess, short


def _read_note(rows):
    counts = rows[3:]
    fields = []
    for start, packed in zip(_list_starts(counts)[0], counts):
        count = (packed >> (3 * _sublane())) & 7
        lo = jnp.where(start < 32, rows[0], jnp.where(start < 64, rows[1], rows[2]))
        hi = jnp.where(start < 32, rows[1], rows[2])
        entries = _shr(lo, start & 31) | ((hi << 1) << (31 - (start & 31)))
        a = b = jnp.zeros((8, 128), I32)
        for j in range(LIST_MAX):
            entry = entries >> (5 * j)
            one = jnp.where(count > j, 1 << ((entry & 15) << 1), 0)
            second = (entry & 16) != 0
            a, b = a + jnp.where(second, 0, one), b + jnp.where(second, one, 0)
        fields += [a, b]
    excess = [_shift(fields[t // 8], 10 - 2 * (t % 8)) & LISTED for t in range(TILES)]
    return excess, _both_halves(_shr(rows[3], 24) | (((rows[4] >> 24) & 0x7F) << 8))


def _tiles(t, n=1):
    return pl.ds(8 * t, 8 * n)


def _runs(cuts):
    return list(zip(cuts[:-1], cuts[1:]))


def _kernel(x_hbm, wq_hbm, kt_hbm, vt_hbm, wo_hbm, out_ref,
            x_f32, wq_f32, wo_f32, k_f32, v_f32, x_bf16, q_own, ctx, acc,
            own, body, note, plane, excess, floors,
            wq_sem, wo_sem, x_sem, kv_sem, send_sem, plane_send_sem, body_sem, note_sem, plane_sem,
            ready_sem):
    me = lax.axis_index("i")
    chip = (me, (me + 3) & 3, (me + 1) & 3, (me + 2) & 3)
    head, late, tail, whole = _runs(HEAD_CUTS), _runs(LATE_CUTS), _runs(TAIL_CUTS), [(0, TILES)]

    def wq_load(h, c):
        rows = pl.ds(16 * head[c][0], 16 * (head[c][1] - head[c][0]))
        cols = pl.ds(pl.multiple_of(h * PAIR, PAIR), PAIR)
        return pltpu.make_async_copy(wq_hbm.at[rows, cols], wq_f32.at[h, rows], wq_sem.at[h * len(head) + c])

    wo_load = pltpu.make_async_copy(wo_hbm, wo_f32, wo_sem)
    x_load = pltpu.make_async_copy(x_hbm, x_f32, x_sem)

    def kv_loads(step):
        copies = []
        for s, h in STEPS[step]:
            src = (pl.ds(me * B_LOC, B_LOC), pl.ds(pl.multiple_of((chip[s] * 2 + h) * PAIR, PAIR), PAIR))
            copies.append(pltpu.make_async_copy(kt_hbm.at[src], k_f32.at[s, h], kv_sem.at[step]))
            copies.append(pltpu.make_async_copy(vt_hbm.at[src], v_f32.at[s, h], kv_sem.at[step]))
        return copies

    def start(*copies):
        for copy in copies:
            copy.start()

    def wait(*copies):
        for copy in copies:
            copy.wait()

    def remote(buf, rows, s, w, h, d, sems, run=0, send=send_sem):
        to = LEFT + d if s == OWN else DIAG
        sem = sems.at[run * 12 + (to - 1) * 4 + w * 2 + h]
        return pltpu.make_async_remote_copy(
            buf.at[(s, w, h, *rows)], buf.at[(to, w, h, *rows)], send, sem,
            device_id=((me + 1 + 2 * d) & 3,), device_id_type=pl.DeviceIdType.MESH)

    def body_copy(s, w, h, d, cut, run=0):
        i0, i1 = (_body_cut(w, t) for t in cut)
        return remote(body, [_tiles(i0, i1 - i0)], s, w, h, d, body_sem, run)

    def note_copy(*route):
        return remote(note, [], *route, note_sem)

    def plane_copy(*route):
        return remote(plane, [], *route, plane_sem, send=plane_send_sem)

    def route_to(s, w, h):
        return (LEFT + h, w, h, h) if s == DIAG else (OWN, w, h, s - LEFT)

    short = {}
    sent, noted = [], []

    def send_body(s, w, h, d, runs):
        for run, cut in enumerate(runs):
            sent.append(body_copy(s, w, h, d, cut, run))
            sent[-1].start()

    def send_note(s, w, h, d):
        noted.append((s, w, h, d))
        sent.append(note_copy(s, w, h, d))
        sent[-1].start()
        pl.when(short[s, w, h])(lambda: plane_copy(s, w, h, d).start())

    def pack_body(w, h, cut):
        for i in range(*(_body_cut(w, t) for t in cut)):
            kept, spread = PLAN[w][i]
            v = own[w, h, _tiles(kept), :] & REST
            for t, n, bits in spread:
                v |= _shift(own[w, h, _tiles(t), :], n) & bits
            body[OWN, w, h, _tiles(i), :] = v

    def write_note(w, h):
        rows, over, short[OWN, w, h] = _make_note([own[w, h, _tiles(t), :] for t in range(TILES)])
        for r, v in enumerate(rows):
            note[OWN, w, h, r:r + 1, :] = v
        for i in range(PLANE_TILES):
            plane[OWN, w, h, _tiles(i), :] = sum(v >> (5 * j) for j, v in enumerate(over[3 * i:3 * i + 3]))

    def wait_notes(pieces):
        for p in pieces:
            note_copy(*route_to(*p)).wait_recv()

    def read_notes(pieces):
        flags = 0
        for i, p in enumerate(pieces):
            rows = [note[(*p, slice(r, r + 1))] for r in range(NOTE_ROWS)]
            over, floors[p] = _read_note(rows)
            excess[p] = jnp.concatenate(over, axis=0)
            flags |= _shr(rows[4], 31) << i
        flags = flags[0, 0]
        for i, p in enumerate(pieces):
            short[p] = ((flags >> i) & 1) == 1

        @pl.when(flags != 0)
        def _():
            for p in pieces:
                @pl.when(short[p])
                def _():
                    plane_copy(*route_to(*p)).wait_recv()
                    for t in range(TILES):
                        excess[(*p, _tiles(t))] = (plane[(*p, _tiles(t // 3))] << (5 * (t % 3))) & HIGH

    def wait_body(s, w, h, runs=whole, run=0):
        body_copy(*route_to(s, w, h), runs[run], run).wait_recv()

    def weights(s, w, h, t0, t1):
        if s == OWN:
            return pltpu.bitcast(own[w, h, _tiles(t0, t1 - t0), :], BF16)
        out = []
        for t in range(t0, t1):
            rest = 0
            for i, (kept, spread) in enumerate(PLAN[w]):
                if kept == t:
                    rest = body[s, w, h, _tiles(i), :] & REST
                for n, bits in [(n, bits) for u, n, bits in spread if u == t]:
                    rest |= _shift(body[s, w, h, _tiles(i), :] & bits, -n)
            out.append(_highest(rest, floors[s, w, h]) - excess[s, w, h, _tiles(t), :])
        return pltpu.bitcast(jnp.concatenate(out, axis=0), BF16)

    def q_proj(step):
        w = jnp.concatenate([weights(s, WQ, h, 0, TILES) for s, h in STEPS[step]], axis=1)
        return jnp.dot(pltpu.bitcast(x_bf16[...], BF16), w, preferred_element_type=F32)

    def attention(step, q):
        low = lax.broadcasted_iota(I32, (BLK, PAIR), 1) < BLK
        low_row = lax.broadcasted_iota(I32, (1, PAIR), 1) < BLK
        scores = {}
        for m in range(TOK // PAIR):
            b, t = divmod(m, SEQ // PAIR)
            for i, (s, h) in enumerate(STEPS[step]):
                q0 = q[m * PAIR:m * PAIR + BLK, i * PAIR:(i + 1) * PAIR]
                q1 = q[m * PAIR + BLK:(m + 1) * PAIR, i * PAIR:(i + 1) * PAIR]
                k = (k_f32[s, h, b, :, t * PAIR:(t + 1) * PAIR] * SCORE_SCALE).T
                for e in range(2):
                    mine = low if e == 0 else jnp.logical_not(low)
                    qe = jnp.concatenate([jnp.where(mine, q0, 0.0), jnp.where(mine, 0.0, q1)], axis=0)
                    ke = jnp.where(mine, k[:BLK], k[BLK:])
                    scores[m, i, e] = lax.dot_general(
                        ke.astype(BF16), qe.astype(BF16), (((1,), (1,)), ((), ())),
                        preferred_element_type=F32)
        for m in range(TOK // PAIR):
            b, t = divmod(m, SEQ // PAIR)
            outs = {}
            for i, (s, h) in enumerate(STEPS[step]):
                p, masked, scale = [], [], []
                for e in range(2):
                    top = jnp.maximum(jnp.max(scores[m, i, e], axis=0, keepdims=True), MASKED_SCORE)
                    p.append(jnp.exp2(scores[m, i, e] - top))
                    masked.append(jnp.exp2(MASKED_SCORE - top))
                    scale.append(1.0 / (jnp.sum(p[e], axis=0, keepdims=True) + (SEQ - BLK) * masked[e]))
                for e in range(2):
                    pe = jnp.concatenate(
                        [jnp.where(low, p[e], masked[1 - e]), jnp.where(low, masked[e], p[1 - e])], axis=0)
                    near = v_f32[s, h, b, e * BLK:(e + 1) * BLK, t * PAIR:(t + 1) * PAIR]
                    far = v_f32[s, h, b, e * BLK:(e + 1) * BLK, (1 - t) * PAIR:(2 - t) * PAIR]
                    o = jnp.dot(near.astype(BF16), pe.astype(BF16), preferred_element_type=F32)
                    o += jnp.sum(far, axis=1, keepdims=True) * jnp.where(low_row, masked[e], masked[1 - e])
                    outs[i, e] = o * jnp.where(low_row, scale[e], scale[1 - e])
            for e in range(2):
                c = jnp.concatenate([outs[0, e], outs[1, e]], axis=0).T.astype(BF16)
                ctx[step, e, m * BLK:(m + 1) * BLK, :] = pltpu.bitcast(c, I32)

    def out_proj(step, t0, t1, dst=acc):
        heads = range(2) if t1 - t0 > 4 else [t0 // 4 % 2]
        blocks = range(t0 // 8, (t1 + 7) // 8)
        cols = slice(blocks[0] * 128, (blocks[-1] + 1) * 128)
        w = jnp.concatenate(
            [jnp.concatenate([weights(s, WO, h, 8 * n + 4 * e, 8 * n + 4 * e + 4) for n in blocks], axis=1)
             for e in heads for s, h in STEPS[step]], axis=0)
        size = TOK // max(1, 4 // (len(heads) * len(blocks)))
        for r in range(0, TOK, size):
            c = jnp.concatenate(
                [pltpu.bitcast(ctx[step, e, r // 2:(r + size) // 2, :], BF16) for e in heads], axis=1)
            res = jnp.dot(c, w, preferred_element_type=F32)
            if step > 0:
                res += acc[r:r + size, cols]
            dst[r:r + size, cols] = res.astype(dst.dtype)

    def signal_neighbours(sem):
        for s in (LEFT, RIGHT):
            pl.semaphore_signal(sem, 1, device_id=(chip[s],), device_id_type=pl.DeviceIdType.MESH)

    def stage_wq(h, c):
        t0, t1 = head[c]
        wq_load(h, c).wait()
        own[WQ, h, _tiles(t0, t1 - t0), :] = pltpu.bitcast(wq_f32[h, 16 * t0:16 * t1, :].astype(BF16), I32)
        pack_body(WQ, h, head[c])

    first = jnp.where(me == 1, 1, 0)
    last = len(head) - 1
    start(*[wq_load(first, c) for c in range(last)])
    barrier = pltpu.get_barrier_semaphore()
    pl.when(me != 2)(lambda: signal_neighbours(barrier))

    @pl.when((me & 1) == 1)
    def _():
        pl.semaphore_wait(barrier, 1)
        for c in range(len(head)):
            stage_wq(first, c)
            body_copy(OWN, WQ, first, first, head[c]).start()
            if c == 0:
                wq_load(first, last).start()
            if c == last - 1:
                start(*[wq_load(1 - first, other) for other in range(len(head))], wo_load, x_load)
        for c in range(len(head)):
            stage_wq(1 - first, c)
        pl.semaphore_wait(ready_sem, 1)
        start(*[body_copy(OWN, WQ, 1 - first, 1 - first, cut) for cut in head])

    @pl.when((me & 1) == 0)
    def _():
        start(*[wq_load(h, c) for c in range(len(head)) for h in range(2) if h == 1 or c == last])
        pl.when(me == 0)(lambda: start(wo_load, x_load))
        pl.semaphore_wait(barrier, 2)
        pl.when(me == 2)(lambda: signal_neighbours(ready_sem))
        for c in range(len(head)):
            for h in range(2):
                stage_wq(h, c)
                body_copy(OWN, WQ, h, h, head[c]).start()
            if c == last - 1:
                pl.when(me == 2)(lambda: start(wo_load, x_load))

    sent += [body_copy(OWN, WQ, h, h, cut) for h in range(2) for cut in head]

    near_q, near_o = ([(LEFT + d, w, h) for d in range(2) for h in range(2)] for w in (WQ, WO))
    far_q, far_o = ([(DIAG, w, h) for h in range(2)] for w in (WQ, WO))

    for h in range(2):
        write_note(WQ, h)
    for d in range(2):
        for h in range(2):
            send_note(OWN, WQ, h, d)
        send_body(OWN, WQ, 1 - d, d, whole)

    wo_load.wait()
    start(*kv_loads(0))
    for h in range(2):
        for n in range(4):
            own[WO, h, _tiles(8 * n, 8), :] = pltpu.bitcast(
                wo_f32[h * PAIR:(h + 1) * PAIR, n * 128:(n + 1) * 128].astype(BF16), I32)
        pack_body(WO, h, whole[0])
        write_note(WO, h)
    for d in range(2):
        for h in range(2):
            send_note(OWN, WO, h, d)
        send_body(OWN, WO, d, d, whole)

    x_load.wait()
    start(*kv_loads(1))
    for b in range(B_LOC):
        x_bf16[b * SEQ // 2:(b + 1) * SEQ // 2, :] = pltpu.bitcast(x_f32[b].astype(BF16), I32)
    q_own[...] = q_proj(0)

    wait_notes(near_q)
    read_notes(near_q)
    for d in range(2):
        wait_body(LEFT + d, WQ, d)
        send_note(LEFT + d, WQ, d, d)
        send_body(LEFT + d, WQ, d, d, whole)
        send_body(OWN, WO, 1 - d, d, late)
    wait(*kv_loads(0))
    start(*kv_loads(2))
    attention(0, q_own)
    out_proj(0, 0, TILES)

    wait(*kv_loads(1))
    start(*kv_loads(3))
    attention(1, q_proj(1))

    for d in range(2):
        wait_body(LEFT + d, WQ, 1 - d)
    wait(*kv_loads(2))
    wait_notes(near_o)
    attention(2, q_proj(2))
    read_notes(near_o)

    for d in range(2):
        wait_body(LEFT + d, WO, d)
        send_note(LEFT + d, WO, d, d)
        send_body(LEFT + d, WO, d, d, tail)
    wait_notes(far_q)
    out_proj(1, 0, TILES)
    read_notes(far_q)

    for p in far_q:
        wait_body(*p)
    wait(*kv_loads(3))
    attention(3, q_proj(3))

    for s, w, h, d in noted:
        pl.when(short[s, w, h])(lambda: plane_copy(s, w, h, d).wait_send())

    for run, cut in enumerate(late):
        for d in range(2):
            wait_body(LEFT + d, WO, 1 - d, late, run)
        if cut[1] == TILES:
            wait_notes(far_o)
        out_proj(2, *cut)
        if cut[1] == TILES:
            read_notes(far_o)

    for run, cut in enumerate(tail):
        for p in far_o:
            wait_body(*p, tail, run)
        out_proj(3, *cut, dst=acc if cut[1] % 8 else out_ref)

    for copy in sent:
        copy.wait_send()


def pallas_dist_sparse_attn_strided_htp_bs_b2_sq256_skv256_hq4_dh64_kernel(x, Wq, K_ext, V_ext, Wo):
    n_b, skv, n_h, dh = K_ext.shape
    kt = K_ext.transpose(0, 2, 3, 1).reshape(n_b, n_h * dh, skv)
    vt = V_ext.transpose(0, 2, 3, 1).reshape(n_b, n_h * dh, skv)
    dma = pltpu.SemaphoreType.DMA
    out = pl.pallas_call(
        _kernel,
        out_shape=jax.ShapeDtypeStruct((TOK, D_MODEL), BF16),
        in_specs=[pl.BlockSpec(memory_space=pltpu.HBM)] * 5,
        out_specs=pl.BlockSpec(memory_space=pltpu.VMEM),
        scratch_shapes=[
            pltpu.VMEM((B_LOC, SEQ, D_MODEL), F32),
            pltpu.VMEM((2, D_MODEL, PAIR), F32),
            pltpu.VMEM((2 * PAIR, D_MODEL), F32),
            pltpu.VMEM((4, 2, B_LOC, PAIR, SEQ), F32),
            pltpu.VMEM((4, 2, B_LOC, PAIR, SEQ), F32),
            pltpu.VMEM((TOK // 2, D_MODEL), I32),
            pltpu.VMEM((TOK, 2 * PAIR), F32),
            pltpu.VMEM((4, 2, TOK // 2, PAIR), I32),
            pltpu.VMEM((TOK, D_MODEL), F32),
            pltpu.VMEM((2, 2, 8 * TILES, 128), I32),
            pltpu.VMEM((4, 2, 2, 8 * BODY_TILES, 128), I32),
            pltpu.VMEM((4, 2, 2, NOTE_ROWS, 128), I32),
            pltpu.VMEM((4, 2, 2, 8 * PLANE_TILES, 128), I32),
            pltpu.VMEM((4, 2, 2, 8 * TILES, 128), I32),
            pltpu.VMEM((4, 2, 2, 8, 128), I32),
            dma((2 * (len(HEAD_CUTS) - 1),)), dma, dma, dma((4,)), dma, dma,
            dma((12 * (len(TAIL_CUTS) - 1),)), dma((12,)), dma((12,)),
            pltpu.SemaphoreType.REGULAR,
        ],
        compiler_params=pltpu.CompilerParams(
            collective_id=0, vmem_limit_bytes=48 * 1024 * 1024,
            disable_semaphore_checks=True),
    )(x, Wq, kt, vt, Wo)
    return out.reshape(x.shape)
```
